```python
import numpy as np

kernel_name = "dist_mlp2_tp_i_m512_h1024_out512"

def setup_inputs():
    x = np.random.randn(512, 512).astype(np.float32)
    W1 = np.random.randn(512, 4096).astype(np.float32)
    W2 = np.random.randn(4096, 512).astype(np.float32)
    return {"x": x, "W1": W1, "W2": W2}

def reference(x: np.ndarray, W1: np.ndarray, W2: np.ndarray) -> np.ndarray:
    h = x @ W1
    h = np.maximum(h, 0.0)
    return h @ W2
```

```python
import functools
import jax, jax.numpy as jnp
from jax import lax
from jax.experimental import pallas as pl
from jax.experimental.pallas import tpu as pltpu

bf = jnp.bfloat16
f32 = jnp.float32
SCOPES = 0
XICI = 1

import contextlib
def scope(name):
    return jax.named_scope(name) if SCOPES else contextlib.nullcontext()

NC = 4
MESH = pl.DeviceIdType.MESH

def pallas_dist_mlp2_tp_i_m512_h1024_out512_kernel(x, W1, W2):
    def body(x_hbm, w1_hbm, w2_hbm, o_ref,
             x_v, w1_v, w2_v, xb, hacc, h, ykeep,
             s1, r1, s2, r2, s3, r3,
             lsem, ssem, rsem, xssem, xrsem):
        i = lax.axis_index("i")
        cx = i >> 1
        cy = (i ^ cx) & 1
        py = i ^ 1
        px = 3 - i
        keep_row = [cx * 128, 256 + cy * 128]
        sent_row = [(1 - cx) * 128, 256 + (1 - cy) * 128]
        peer13 = [px, py]
        peer2 = [py, px]

        bar = pltpu.get_barrier_semaphore()
        for p in (px, py):
            pl.semaphore_signal(bar, inc=1, device_id=(p,), device_id_type=MESH)

        def xcp(slot, row):
            return pltpu.make_async_copy(x_hbm.at[pl.ds(pl.multiple_of(row, 128), 128), :], x_v.at[pl.ds(slot * 128, 128), :], lsem.at[slot])
        xs = [xcp(0, sent_row[0]), xcp(1, sent_row[1])]
        xk = [] if XICI else [xcp(2, keep_row[0]), xcp(3, keep_row[1])]
        w1c = [pltpu.make_async_copy(w1_hbm.at[pl.ds(k * 128, 128), :], w1_v.at[pl.ds(k * 128, 128), :], lsem.at[4 + k]) for k in range(4)]
        w2c0 = [pltpu.make_async_copy(w2_hbm.at[pl.ds(k * 512, 512), pl.ds(0, 128)], w2_v.at[0, pl.ds(k * 512, 512), :], lsem.at[8 + k]) for k in range(2)]
        w2c = [None] + [pltpu.make_async_copy(w2_hbm.at[:, pl.ds(c * 128, 128)], w2_v.at[c], lsem.at[9 + c]) for c in range(1, 4)]

        for c in xs: c.start()
        if not XICI:
            for c in xk: c.start()
        for c in w1c: c.start()
        for c in w2c0: c.start()
        for c in w2c[1:]: c.start()

        def rdma(src, dst, step, g, c, peer):
            return pltpu.make_async_remote_copy(src.at[g, c], dst.at[g, c], ssem.at[step, g, c], rsem.at[step, g, c],
                                                device_id=(peer,), device_id_type=MESH)
        S1 = [[rdma(s1, r1, 0, g, c, peer13[g]) for c in range(NC)] for g in range(2)]
        S2 = [[rdma(s2, r2, 1, g, c, peer2[g]) for c in range(NC)] for g in range(2)]
        S3 = [[rdma(s3, r3, 2, g, c, peer13[g]) for c in range(NC)] for g in range(2)]
        XX = [[pltpu.make_async_remote_copy(xb.at[pl.ds(g * 128 + hh * 64, 64), :], xb.at[pl.ds(256 + hh * 128 + g * 64, 64), :],
                                            xssem.at[g, hh], xrsem.at[g, hh], device_id=(peer13[g],), device_id_type=MESH)
               for hh in range(2)] for g in range(2)]

        with scope("wait_x"):
            for c in xs: c.wait()
        xb[0:256, :] = x_v[0:256, :].astype(bf)
        if XICI:
            with scope("barrier"):
                pl.semaphore_wait(bar, 2)
            for hh in range(2):
                for g in range(2):
                    XX[g][hh].start()
        else:
            for c in xk: c.wait()
            xb[256:512, :] = x_v[256:512, :].astype(bf)

        R = 256 if XICI else 512
        for k in range(4):
            with scope(f"wait_w1_{k}"):
                w1c[k].wait()
            with scope(f"h_{k}"):
                part = jnp.dot(xb[0:R, k * 128:(k + 1) * 128], w1_v[k * 128:(k + 1) * 128, :].astype(bf), preferred_element_type=f32)
                if k == 0:
                    hacc[0:R, :] = part
                elif k < 3:
                    hacc[0:R, :] += part
                else:
                    h[0:R, :] = jnp.maximum(hacc[0:R, :] + part, 0).astype(bf)

        def y_sent(c):
            if c == 0:
                with scope("wait_w2_0a"):
                    w2c0[0].wait()
                with scope("ys_0a"):
                    p0 = jnp.dot(h[0:256, 0:512], w2_v[0, 0:512, :].astype(bf), preferred_element_type=f32)
                    hacc[0:256, 0:128] = p0
                with scope("wait_w2_0b"):
                    w2c0[1].wait()
                with scope("ys_0b"):
                    y = hacc[0:256, 0:128] + jnp.dot(h[0:256, 512:1024], w2_v[0, 512:1024, :].astype(bf), preferred_element_type=f32)
                    s1[0, 0] = y[0:128].astype(bf)
                    s1[1, 0] = y[128:256].astype(bf)
                if not XICI:
                    with scope("barrier"):
                        pl.semaphore_wait(bar, 2)
            else:
                with scope(f"wait_w2_{c}"):
                    w2c[c].wait()
                with scope(f"ys_{c}"):
                    y = jnp.dot(h[0:256, :], w2_v[c].astype(bf), preferred_element_type=f32)
                    s1[0, c] = y[0:128].astype(bf)
                    s1[1, c] = y[128:256].astype(bf)
            for g in range(2):
                S1[g][c].start()

        def h_kept(hh):
            with scope(f"wait_xk_{hh}"):
                for g in range(2):
                    XX[g][hh].wait_recv()
            with scope(f"hk_{hh}"):
                r0 = 256 + hh * 128
                hk = jnp.maximum(jnp.dot(xb[r0:r0 + 128, :], w1_v[...].astype(bf), preferred_element_type=f32), 0).astype(bf)
                h[256 + hh * 64:256 + hh * 64 + 64, :] = hk[0:64]
                h[384 + hh * 64:384 + hh * 64 + 64, :] = hk[64:128]

        def y_kept(c):
            with scope(f"yk_{c}"):
                ykeep[c] = jnp.dot(h[256:512, :], w2_v[c].astype(bf), preferred_element_type=f32)

        def step2(c):
            with scope(f"wait_r1_{c}"):
                for g in range(2):
                    S1[g][c].wait_recv()
            for g in range(2):
                v = ykeep[c, g * 128:(g + 1) * 128, :] + r1[g, c].astype(f32)
                ykeep[c, g * 128:(g + 1) * 128, :] = v
                s2[g, c] = v.astype(bf)
                S2[g][c].start()

        def step3(c):
            with scope(f"wait_r2_{c}"):
                for g in range(2):
                    S2[g][c].wait_recv()
            for g in range(2):
                v = ykeep[c, g * 128:(g + 1) * 128, :] + r2[g, c].astype(f32)
                s3[g, c] = v.astype(bf)
                S3[g][c].start()
                o_ref[pl.ds(pl.multiple_of(keep_row[g], 128), 128), c * 128:(c + 1) * 128] = v

        def fin(c):
            with scope(f"wait_r3_{c}"):
                for g in range(2):
                    S3[g][c].wait_recv()
            for g in range(2):
                o_ref[pl.ds(pl.multiple_of(sent_row[g], 128), 128), c * 128:(c + 1) * 128] = r3[g, c].astype(f32)

        if XICI:
            y_sent(0)
            h_kept(0)
            y_sent(1)
            h_kept(1)
            y_sent(2)
            y_kept(0)
            step2(0)
            y_sent(3)
            y_kept(1)
            step2(1)
            y_kept(2)
            step2(2)
            y_kept(3)
            step2(3)
        else:
            y_sent(0)
            y_kept(0)
            y_sent(1)
            y_kept(1)
            y_sent(2)
            y_kept(2)
            step2(0)
            y_sent(3)
            y_kept(3)
            step2(1)
            step2(2)
            step2(3)
        for c in range(NC):
            step3(c)
        for c in range(NC):
            fin(c)
        with scope("wait_send"):
            for S in (S1, S2, S3):
                for g in range(2):
                    for c in range(NC):
                        S[g][c].wait_send()
            if XICI:
                for g in range(2):
                    for hh in range(2):
                        XX[g][hh].wait_send()

    cb = lambda: pltpu.VMEM((2, NC, 128, 128), bf)
    return pl.pallas_call(
        body,
        out_shape=jax.ShapeDtypeStruct((512, 512), f32),
        in_specs=[pl.BlockSpec(memory_space=pl.ANY)] * 3,
        out_specs=pl.BlockSpec(memory_space=pltpu.VMEM),
        scratch_shapes=[pltpu.VMEM((512, 512), f32), pltpu.VMEM((512, 1024), f32), pltpu.VMEM((NC, 1024, 128), f32),
                        pltpu.VMEM((512, 512), bf), pltpu.VMEM((512, 1024), f32), pltpu.VMEM((512, 1024), bf),
                        pltpu.VMEM((NC, 256, 128), f32),
                        cb(), cb(), cb(), cb(), cb(), cb(),
                        pltpu.SemaphoreType.DMA((13,)), pltpu.SemaphoreType.DMA((3, 2, NC)), pltpu.SemaphoreType.DMA((3, 2, NC)),
                        pltpu.SemaphoreType.DMA((2, 2)), pltpu.SemaphoreType.DMA((2, 2))],
        compiler_params=pltpu.CompilerParams(collective_id=0, vmem_limit_bytes=64 * 1024 * 1024, disable_semaphore_checks=True),
    )(x, W1, W2)
```

```python
import functools

import jax
import jax.numpy as jnp
from jax import lax
from jax.experimental import pallas as pl
from jax.experimental.pallas import tpu as pltpu

SIZES = (48, 48, 48, 48, 32, 32)
UP = "EEELELELEELLLLLLLLLLLLLL"
DOWN = "EEELELELEELLEELLEEEELLLL"
LOADS = {
    "E": "x30 w20 x10 x40 w10 w00 w30 v10 v11 v30 v31 v21 v20 x50 x00 v01 v00",
    "M": "x80 x70 w00 w10 w20 w30 v10 v11 v00 v01 v21 v20 v30 v31 x50 x30 xb0 x40",
    "L": "x00 w00 w10 w20 w30 v00 v01 v11 v10 v20 v21 x40 x50 v30 v31",
}
PROGRAM = {
    "E": (
        "|H320 |X310 X100 X311 H120 X312 |X412 |H410 X410 X313 H110 X413 X411 |H100 H400 H300 X102 H310 H420 "
        "X103 |H330 H430 H130 X101 |Y110 Y310 |Y111 Y410 T110 H210 Y411 H200 Y311 T310 |Y131 Y130 H220 H230 "
        "T130 Y331 Y211 Y330 T410 Y430 Y431 Y231 T330 T430 |Y320 H510 Y321 Y421 Y221 Y230 T320 H500 Y220 T230 "
        "H530 Y420 Y210 H520 |T210 T420 Y520 Y301 Y300 Y531 Y500 Y521 Y530 Y200 T530 Y501 T520 T220 Y201 Y101 "
        "H030 T500 H000 Y401 |T200 Y121 H020 T300 H010 Y400 Y120 Y011 Y010 Y030 T400 |T120 Y001 Y031 T030 "
        "Y100 Y021 T100 Y511 Y000 T000 T010 |U210 Y510 T510 U200 Y020 |U110 U000 T020 U010 U020 |J000 |U300 "
        "U310 U100 |U220 |U030 |U410 U120 |U420 U130 U320 U330 |U400 |U430 |U510 U530 U500 U230 |U520 "
    ),
    "M": (
        "|X820 X720 X803 X721 X822 X801 |H800 X800 H700 X821 X722 X823 X723 |H900 |H810 H100 H710 X802 |H610 "
        "H910 |H600 X922 X921 |Ha20 H920 H720 H820 |H010 Ha00 H000 X920 |Ha30 H020 H930 H830 H730 X923 |Ha10 "
        "Y810 Y910 Ya10 H120 |Y811 Ya11 Y911 Y710 H630 R410 R210 R310 Y711 H620 H030 Y611 Y610 H130 Y011 R010 "
        "R110 |Ya01 Y600 Ya00 Y601 Y900 Y901 Y801 R000 R400 Y800 H110 Y701 R200 R300 Y700 Y110 Y111 H200 H220 "
        "R100 L110 |Y820 Y720 Y821 Y721 Y621 Ya20 Y620 R220 R120 Ya21 Y101 H210 R420 R020 Y000 Y920 Y001 Y921 "
        "Y100 H230 R320 |E000 Y831 Y201 Y830 Y631 Y630 Y200 R230 E001 R030 |E201 E200 |E100 Y931 Y211 Y930 "
        "Y731 Y010 Y730 Y230 R330 R130 |E101 E010 Y231 Y210 Hb00 H300 H320 E011 L230 |E211 E210 |E110 Y020 "
        "Ya31 Hb10 Ya30 Hb20 Y021 Hb30 R430 L210 |E021 E020 Y120 H330 Yb31 Yb30 H310 Y121 E111 R530 |E121 "
        "E120 Y310 Y311 Yb01 Yb00 Yb20 L310 |E311 R500 E310 Y300 Yb11 Yb10 Y301 R510 |E301 E300 Y321 Y220 "
        "Yb21 Y221 R520 |E221 E220 Y320 Y330 H530 L220 L320 L200 |E321 E320 Y331 H400 Y031 L330 |E231 E230 "
        "Y131 H410 H430 H420 |E330 |E331 Y030 Y421 Y410 Y411 L030 |E030 |E031 Y130 Y400 H520 L130 |E411 E410 "
        "Y401 |E130 |E131 Y430 Y420 H500 H510 L410 L420 |E420 E421 |E400 |E401 Y500 Y530 Y531 Y501 Y431 L530 "
        "L500 |E430 E431 |E530 Y511 Y510 Y520 Y521 L510 F210 |E500 L520 E531 L300 |E501 L120 L000 |E510 F200 "
        "|E511 |E520 |E521 L400 L430 |J000 L010 L020 |F100 L100 |F130 F020 F230 F420 F010 F000 F120 |F530 "
        "F220 |F430 F400 |F500 F410 F330 F320 F110 F030 F300 F310 |F510 |F520 "
    ),
    "L": (
        "|X011 |X010 X000 X001 X002 X003 |H000 |H200 X012 |H010 X013 X200 |H110 H100 |X202 |H020 H220 |H120 "
        "H210 X201 |X203 H030 H230 |Y000 H130 |Y001 Y200 T000 Y101 Y201 Y100 T200 |Y211 Y011 T100 |Y010 H310 "
        "T010 Y210 H300 T210 Y110 Y111 |T110 Y020 Y021 Y121 Y120 T020 H320 T120 H330 Y220 Y310 Y311 Y301 T310 "
        "Y300 Y221 |T300 T220 Y230 Y030 Y231 Y321 Y330 Y320 |T320 |T230 Y331 H410 Y031 H420 H430 |T330 T030 "
        "Y131 H400 Y130 Y411 Y421 Y410 Y431 Y420 T410 |T130 Y400 Y401 T420 H520 Y430 H530 H510 T400 H500 "
        "|T430 Y531 Y530 Y501 Y500 T530 |T500 Y510 Y520 Y511 U310 |T510 Y521 U210 |T520 U110 U230 |U320 U220 "
        "|U330 |U030 |U130 |U530 U420 |U500 U410 |U510 |U520 |J000 |U300 |U010 U400 U120 U000 |U020 U430 U200 "
        "|U100 "
    ),
}

bf16 = jnp.bfloat16
f32 = jnp.float32
MESH = pl.DeviceIdType.MESH
POS_E, POS_M, POS_L = 0, (1, 3), 2

NP = len(SIZES)
NU = 4 * NP
OFF = [2 * sum(SIZES[:p]) for p in range(NP)]
PIECE = [(s // 2 + 15) // 16 * 16 for s in SIZES]
REG = 2 * max(SIZES)
G2 = 4
QLIM = 27
AGE = 128


def _parse(text):
    return [(t.lstrip("|")[0], *(int(d, 16) for d in t.lstrip("|")[1:]), t[0] == "|") for t in text.split()]


def _split_units():
    group, where = 0, {}
    for ty, b, c, hh, new in _parse(PROGRAM["M"]):
        group += new
        if ty == "E":
            where[(b * 4 + c, hh)] = group
    return [where[(u, 0)] != where[(u, 1)] for u in range(NU)]


SPLIT = _split_units()


def _wait(ref, sem):
    pltpu.make_async_copy(ref, ref, sem).wait()


def _piece(b, u, hh):
    if not SPLIT[u]:
        return 0, SIZES[b]
    return (0, PIECE[b]) if hh == 0 else (PIECE[b], SIZES[b] - PIECE[b])


class _Role:
    def __init__(self, pos, refs, barrier):
        (self.x_hbm, self.w1_hbm, self.w2_hbm, self.o, self.x_v, self.w1_v, self.w2_v, self.xb,
         self.hacc, self.h, self.sbuf, self.rbuf, self.lsem, self.ssem, self.rsem, self.xssem,
         self.xrsem) = refs
        self.barrier = barrier
        self.pos = pos
        self.node = "E" if pos == POS_E else "L" if pos == POS_L else "M"
        self.j = POS_M.index(pos) if self.node == "M" else None
        self.loads = [t[:3] for t in _parse(LOADS[self.node])]
        self.issued, self.waited = 0, -1
        self.ready = set()
        self.hcount, self.ycount, self.core_done = {}, {}, {}
        self.pending = []
        self.sent_rows = self.xsent_rows = 0
        prog, seen = [], set()
        for t in _parse(PROGRAM[self.node]):
            if t[0] == "E" and not SPLIT[t[1] * 4 + t[2]]:
                if t[1:3] in seen:
                    continue
                seen.add(t[1:3])
            prog.append(t)
        self.early = (prog[0][1], prog[0][3]) if self.node == "L" else (None, None)
        k = [t[0] for t in prog].index("J")
        self.parts = (prog[:k], prog[k + 1:])

    def half(self, b):
        return self.j if b < NP else 1 - self.j

    def rows(self, b):
        p = b % NP
        if self.node == "M":
            return OFF[p] + self.half(b) * SIZES[p], SIZES[p]
        return OFF[p], 2 * SIZES[p]

    def load_early(self, first):
        b, k = self.early
        rows = pl.ds(*self.rows(b))
        cols = [(0, k * 128, 128)] if first else [(1, 0, k * 128), (2, k * 128 + 128, 384 - k * 128)]
        return [pltpu.make_async_copy(self.x_hbm.at[rows, pl.ds(c0, n)], self.x_v.at[rows, pl.ds(c0, n)],
                                      self.lsem.at[12 + NP + q]) for q, c0, n in cols if n]

    def load(self, kind, a, hh):
        if kind == "x" and a == self.early[0]:
            return self.load_early(True) + self.load_early(False)
        if kind == "x":
            rows = pl.ds(*self.rows(a))
            return [pltpu.make_async_copy(self.x_hbm.at[rows, :], self.x_v.at[rows, :], self.lsem.at[12 + a])]
        if kind == "w":
            rows = pl.ds(a * 128, 128)
            return [pltpu.make_async_copy(self.w1_hbm.at[rows, :], self.w1_v.at[rows, :], self.lsem.at[a])]
        outer = pl.ds(hh * (64 // G2), 64 // G2)
        return [pltpu.make_async_copy(self.w2_hbm.at[outer, pl.ds(q * 8, 8), pl.ds(a * 128, 128)],
                                      self.w2_v.at[a, outer, pl.ds(q * 8, 8), :],
                                      self.lsem.at[4 + 2 * a + hh]) for q in range(G2)]

    def issue_loads(self, upto=-1):
        def in_flight():
            return sum(G2 if t[0] == "v" else 3 if t[:2] == ("x", self.early[0]) else 1
                       for t in self.loads[self.waited + 1:self.issued + 1])

        while self.issued < len(self.loads) and (self.issued <= upto or in_flight() <= QLIM):
            for cp in self.load(*self.loads[self.issued]):
                cp.start()
            self.issued += 1

    def wait_load(self, kind, a, hh):
        if (kind, a, hh) in self.ready:
            return False
        self.ready.add((kind, a, hh))
        i = self.loads.index((kind, a, hh))
        self.issue_loads(upto=i)
        self.waited = max(self.waited, i)
        if kind == "v":
            _wait(self.w2_v.at[a, pl.ds(hh * (64 // G2), 64 // G2)], self.lsem.at[4 + 2 * a + hh])
        else:
            self.load(kind, a, hh)[0].wait()
        return True

    def wait_x(self, b, k):
        if b == self.early[0]:
            first = k == self.early[1]
            if ("early", first) not in self.ready:
                self.ready.add(("early", first))
                for cp in self.load_early(first):
                    cp.wait()
                self.cast_x(b, [q for q in range(4) if (q == self.early[1]) == first])
            return False
        if ("x", b, 0) in self.loads:
            return self.wait_load("x", b, 0)
        if ("X", b, k) not in self.ready:
            self.ready.add(("X", b, k))
            q = (b % NP) * 2 + (self.half(b) if self.node == "M" else 0)
            _wait(self.xb.at[k, pl.ds(*self.rows(b)), :], self.xrsem.at[q * 4 + k])
        return False

    def cast_x(self, b, chunks=range(4)):
        r0, n = self.rows(b)
        for k in chunks:
            self.xb[k, r0:r0 + n, :] = self.x_v[r0:r0 + n, k * 128:(k + 1) * 128].astype(bf16)

    def send_x(self, p, half, k, dest):
        ref = self.xb.at[k, pl.ds(OFF[p] + half * SIZES[p], SIZES[p]), :]
        q = p * 2 + (half if dest in POS_M else 0)
        pltpu.make_async_remote_copy(ref, ref, self.xssem, self.xrsem.at[q * 4 + k],
                                     device_id=(dest,), device_id_type=MESH).start()
        self.xsent_rows += SIZES[p]

    def send(self, src, dst, n, sem, dest):
        pltpu.make_async_remote_copy(self.sbuf.at[pl.ds(src, n), :], self.rbuf.at[pl.ds(dst, n), :],
                                     self.ssem, self.rsem.at[sem],
                                     device_id=(dest,), device_id_type=MESH).start()
        self.sent_rows += n

    def store(self, t):
        ty, b, c, part = t["ty"], t["b"], t["c"], t["val"]
        r0, n = self.rows(b)
        if ty == "H":
            done = self.hcount.get(b, 0)
            self.hcount[b] = done + 1
            if done:
                part = self.hacc[r0:r0 + n, :] + part
            if done == 3:
                self.h[r0:r0 + n, :] = jnp.maximum(part, 0).astype(bf16)
            else:
                self.hacc[r0:r0 + n, :] = part
            return
        cols = slice(c * 128, (c + 1) * 128)
        u = (b % NP) * 4 + c
        done = self.ycount.get((b, c), 0)
        self.ycount[(b, c)] = done + t["halves"]
        final = done + t["halves"] == 2
        leaf = self.node == "M" and b >= NP
        if done:
            part = self.o[r0:r0 + n, cols] + part
        if final and leaf:
            self.sbuf[(NU + u) * REG:(NU + u) * REG + n, :] = part.astype(bf16)
            return
        self.o[r0:r0 + n, cols] = part
        if final and self.node != "M" and UP[u] != self.node:
            self.sbuf[u * REG:u * REG + n, :] = part.astype(bf16)

    def flush(self, pred):
        last = max([i for i, t in enumerate(self.pending) if pred(t)], default=-1)
        for t in self.pending[:last + 1]:
            self.store(t)
        self.pending = self.pending[last + 1:]

    def matmul(self, ty, b, c, halves):
        r0, n = self.rows(b)
        if ty == "H":
            lhs, w = self.xb[c, r0:r0 + n, :], self.w1_v[c * 128:(c + 1) * 128, :]
            cycles = 2 * n
        else:
            self.flush(lambda t: t["ty"] == "H" and t["b"] == b)
            k0, k1 = min(halves) * 512, (max(halves) + 1) * 512
            lhs = self.h[r0:r0 + n, k0:k1]
            w = self.w2_v[c, k0 // (8 * G2):k1 // (8 * G2)].reshape(k1 - k0, 128)
            cycles = len(halves) * n
        val = jnp.dot(lhs, w.astype(bf16), preferred_element_type=f32)
        for t in self.pending:
            t["age"] += cycles
        self.pending.append(dict(ty=ty, b=b, c=c, val=val, halves=len(halves), age=0))
        self.flush(lambda t: t["age"] >= AGE)

    def waits(self, tasks):
        casts = []
        if "barrier" in self.ready and tasks[0][0] not in "HYX":
            tasks = tasks[1:] + tasks[:1]
        for ty, b, c, hh, _ in tasks:
            if ty == "H":
                if self.wait_x(b, c):
                    casts.append(b)
                self.wait_load("w", c, 0)
            elif ty == "Y":
                self.wait_load("v", c, hh)
            elif ty == "X":
                if self.wait_x(b, hh):
                    if "barrier" in self.ready:
                        casts.append(b)
                    else:
                        self.cast_x(b)
            else:
                u, s = b * 4 + c, SIZES[b]
                lo, hi = u * REG, (NU + u) * REG
                if ty == "T" and UP[u] == self.node:
                    _wait(self.rbuf.at[pl.ds(lo, 2 * s), :], self.rsem.at[2 * u])
                elif ty == "U":
                    _wait(self.rbuf.at[pl.ds(hi, 2 * s), :], self.rsem.at[2 * (NU + u)])
                elif ty == "E":
                    q0, m = _piece(b, u, hh)
                    _wait(self.rbuf.at[pl.ds(lo + s + q0, m), :],
                          self.rsem.at[2 * u + 1 + (2 * NU if q0 else 0)])
                elif ty == "L":
                    _wait(self.rbuf.at[pl.ds(lo, s), :], self.rsem.at[2 * u])
                elif ty == "F":
                    _wait(self.rbuf.at[pl.ds(hi, s), :], self.rsem.at[2 * (NU + u)])
            if ty not in "HY" and "barrier" not in self.ready:
                self.ready.add("barrier")
                pl.semaphore_wait(self.barrier, 2)
        for b in casts:
            self.cast_x(b)

    def message(self, ty, b, c, hh):
        if ty == "X":
            if self.node == "M":
                self.send_x(b % NP, self.half(b), hh, POS_E if c == 0 else POS_L)
            else:
                for j in range(2):
                    self.send_x(b, j if c == 0 else 1 - j, hh, POS_M[j])
            return
        o, sbuf, rbuf = self.o, self.sbuf, self.rbuf
        u, s = b * 4 + c, SIZES[b]
        lo, hi = u * REG, (NU + u) * REG
        cols = slice(c * 128, (c + 1) * 128)
        yb = b + NP if ty in "RF" else b
        self.flush(lambda t: t["ty"] == "Y" and (t["b"], t["c"]) == (yb, c))
        r0, n = self.rows(yb)
        if ty == "T":
            if UP[u] == self.node:
                v = o[r0:r0 + n, cols] + rbuf[lo:lo + n, :].astype(f32)
                o[r0:r0 + n, cols] = v
                sbuf[lo:lo + n, :] = v.astype(bf16)
            if self.node == "E":
                for j in range(2):
                    self.send(lo + j * s, lo, s, 2 * u, POS_M[j])
            else:
                for q in range(2 if SPLIT[u] else 1):
                    q0, m = _piece(b, u, q)
                    for j in range(2):
                        self.send(lo + j * s + q0, lo + s + q0, m, 2 * u + 1 + 2 * NU * q, POS_M[j])
        elif ty == "U":
            v = o[r0:r0 + n, cols] + rbuf[hi:hi + n, :].astype(f32)
            o[r0:r0 + n, cols] = v
            if DOWN[u] == self.node:
                sbuf[hi:hi + n, :] = v.astype(bf16)
                for j in range(2):
                    self.send(hi + j * s, hi, s, 2 * (NU + u), POS_M[1 - j])
        elif ty == "R":
            self.send(hi, lo + (1 - self.j) * s, s, 2 * u, POS_E if UP[u] == "E" else POS_L)
        elif ty == "E":
            done = self.core_done.setdefault(u, [])
            q0, m = _piece(b, u, hh)
            v = o[r0 + q0:r0 + q0 + m, cols] + rbuf[lo + s + q0:lo + s + q0 + m, :].astype(f32)
            sbuf[lo + q0:lo + q0 + m, :] = v.astype(bf16)
            if "L" in done:
                o[r0 + q0:r0 + q0 + m, cols] = v + rbuf[lo + q0:lo + q0 + m, :].astype(f32)
            done.append((q0, m))
            self.send(lo + q0, hi + self.j * s + q0, m, 2 * (NU + u), POS_E)
        elif ty == "L":
            done = self.core_done.setdefault(u, [])
            v = o[r0:r0 + s, cols] + rbuf[lo:lo + s, :].astype(f32)
            sbuf[lo + s:lo + 2 * s, :] = v.astype(bf16)
            for q0, m in sorted(done):
                o[r0 + q0:r0 + q0 + m, cols] = v[q0:q0 + m] + rbuf[lo + s + q0:lo + s + q0 + m, :].astype(f32)
            done.append("L")
            self.send(lo + s, hi + self.j * s, s, 2 * (NU + u), POS_L)
        elif ty == "F":
            o[r0:r0 + s, cols] = rbuf[hi:hi + s, :].astype(f32)

    def run(self, part):
        prog = self.parts[part]
        starts = [i for i, t in enumerate(prog) if t[4] or i == 0] + [len(prog)]
        for i, k in zip(starts, starts[1:]):
            grp = prog[i:k]
            self.waits(grp)
            lead = next((q for q, t in enumerate(grp) if t[0] in "HY"), 0)
            if lead and grp[lead][0] == "Y":
                grp = [grp[lead]] + grp[:lead] + grp[lead + 1:]
            q = 0
            while q < len(grp):
                ty, b, c, hh, _ = grp[q]
                if ty == "Y" and self.node == "M" and q + 1 < len(grp) and grp[q + 1][:3] == (ty, b, c):
                    self.matmul(ty, b, c, [0, 1])
                    q += 1
                elif ty in "HY":
                    self.matmul(ty, b, c, [hh])
                else:
                    self.message(ty, b, c, hh)
                q += 1
            self.issue_loads()
            self.flush(lambda t: True)
        if part == 1:
            _wait(self.sbuf.at[pl.ds(0, self.sent_rows), :], self.ssem)
            if self.xsent_rows:
                _wait(self.sbuf.at[pl.ds(0, self.xsent_rows), :], self.xssem)


def _body(*refs):
    me = lax.axis_index("i")
    barrier = pltpu.get_barrier_semaphore()
    for nbr in (me ^ 1, 3 - me):
        pl.semaphore_signal(barrier, inc=1, device_id=(nbr,), device_id_type=MESH)
    roles = [_Role(pos, refs, barrier) for pos in range(4)]
    for r in roles:
        pl.when(me == r.pos)(r.issue_loads)
    for part in range(2):
        for r in roles:
            pl.when(me == r.pos)(functools.partial(r.run, part))


def pallas_dist_mlp2_tp_i_m512_h1024_out512_kernel(x: jax.Array, W1: jax.Array, W2: jax.Array):
    return pl.pallas_call(
        _body,
        out_shape=jax.ShapeDtypeStruct((512, 512), f32),
        in_specs=[pl.BlockSpec(memory_space=pl.ANY)] * 3,
        out_specs=pl.BlockSpec(memory_space=pltpu.VMEM),
        scratch_shapes=[
            pltpu.VMEM((512, 512), f32),
            pltpu.VMEM((512, 1024), f32),
            pltpu.VMEM((4, 128 // G2, 8 * G2, 128), f32),
            pltpu.VMEM((4, 512, 128), bf16),
            pltpu.VMEM((512, 1024), f32),
            pltpu.VMEM((512, 1024), bf16),
            pltpu.VMEM((2 * NU * REG, 128), bf16),
            pltpu.VMEM((2 * NU * REG, 128), bf16),
            pltpu.SemaphoreType.DMA((12 + 2 * NP,)),
            pltpu.SemaphoreType.DMA,
            pltpu.SemaphoreType.DMA((4 * NU,)),
            pltpu.SemaphoreType.DMA,
            pltpu.SemaphoreType.DMA((8 * NP,)),
        ],
        compiler_params=pltpu.CompilerParams(
            collective_id=0, vmem_limit_bytes=64 * 1024 * 1024, disable_semaphore_checks=True),
    )(x, W1, W2.reshape(128 // G2, 8 * G2, 512))
```
